```python
import numpy as np

kernel_name = "dist_mean_ax1_xy_m1024_n512"

def setup_inputs():
    return {"x": np.random.randn(2048, 1024).astype(np.float32)}

def reference(x: np.ndarray) -> np.ndarray:
    return np.mean(x, axis=1, keepdims=True)
```

```python
import jax
import jax.numpy as jnp
from jax import lax
from jax.experimental import pallas as pl
from jax.experimental.pallas import tpu as pltpu

LANES = 128
SUBLANES = 8
Y_SIZE = 2

CHUNKS = (256, 384, 128, 128, 88, 40)
PRIORITIES = (0, 0, 0, 0, 1, 1)
MESSAGES = (5, 2, 1)


def pallas_dist_mean_ax1_xy_m1024_n512_kernel(x: jax.Array):
    m, n = x.shape
    groups = m // LANES
    streamed = CHUNKS[-1]
    assert sum(CHUNKS) == m and sum(MESSAGES) == groups and MESSAGES[-1] == 1
    assert n == 4 * LANES and streamed < LANES
    scale = 1.0 / (Y_SIZE * n)

    def body(x_hbm, out_ref, x_buf, raw_buf, part, recv,
             load_sems, send_sems, recv_sems, raw_send_sem, raw_recv_sem):
        loads = []
        row0 = 0
        for i, rows in enumerate(CHUNKS):
            load = pltpu.make_async_copy(
                x_hbm.at[pl.ds(row0, rows)], x_buf.at[pl.ds(row0, rows)],
                load_sems.at[i])
            load.start(priority=PRIORITIES[i])
            loads.append(load)
            row0 += rows

        my_y = lax.axis_index("y")
        peer = (lax.axis_index("x"), 1 - my_y)
        is_streamer = my_y == 1
        is_helper = my_y == 0
        barrier = pltpu.get_barrier_semaphore()
        pl.semaphore_signal(barrier, 1, device_id=peer,
                            device_id_type=pl.DeviceIdType.MESH)

        raw = pltpu.make_async_remote_copy(
            x_hbm.at[pl.ds(m - streamed, streamed)], raw_buf,
            raw_send_sem, raw_recv_sem,
            device_id=peer, device_id_type=pl.DeviceIdType.MESH)

        @pl.when(is_streamer)
        def _():
            pl.semaphore_wait(barrier, 1)
            raw.start()

        messages = []
        group0 = 0
        for j, count in enumerate(MESSAGES):
            messages.append((group0, count, pltpu.make_async_remote_copy(
                part.at[pl.ds(group0, count)], recv.at[pl.ds(group0, count)],
                send_sems.at[j], recv_sems.at[j],
                device_id=peer, device_id_type=pl.DeviceIdType.MESH)))
            group0 += count
        message_ending_at = {
            (g0 + count) * LANES: j for j, (g0, count, _) in enumerate(messages)}
        last_message = messages[-1][2]

        lane = lax.broadcasted_iota(jnp.int32, (SUBLANES, LANES), 1)
        lane_hi = lane >> 3
        lane_lo = lane & 7

        def merge(acc, block, row):
            folded = ((block[:, 0 * LANES:1 * LANES] + block[:, 1 * LANES:2 * LANES])
                      + (block[:, 2 * LANES:3 * LANES] + block[:, 3 * LANES:4 * LANES]))
            sums = jnp.broadcast_to(
                jnp.sum(folded, axis=1, keepdims=True), (SUBLANES, LANES))
            if acc is None:
                return sums
            return jnp.where(lane_hi == (row % LANES) // SUBLANES, sums, acc)

        def to_row(acc):
            return jnp.take_along_axis(acc, lane_lo, axis=0)[0:1]

        acc = None
        own = {}
        row0 = 0
        for i, rows in enumerate(CHUNKS):
            loads[i].wait()
            for r in range(row0, row0 + rows, SUBLANES):
                acc = merge(None if r % LANES == 0 else acc,
                            x_buf[pl.ds(r, SUBLANES), :], r)
                done = r + SUBLANES
                if done == m - streamed:
                    early_row = to_row(acc)

                    @pl.when(is_streamer)
                    def _():
                        part[groups - 1] = early_row
                        last_message.start()

                if done % LANES:
                    continue
                g = r // LANES
                own[g] = to_row(acc)
                if done == m:
                    @pl.when(is_helper)
                    def _():
                        part[g] = own[g]
                        last_message.start()
                    continue
                part[g] = own[g]
                if done in message_ending_at:
                    j = message_ending_at[done]
                    if j == 0:
                        @pl.when(is_helper)
                        def _():
                            pl.semaphore_wait(barrier, 1)
                    messages[j][2].start()
            row0 += rows

        def finish(j):
            g0, count, message = messages[j]
            message.wait_recv()
            for g in range(g0, g0 + count):
                out_ref[:, pl.ds(g * LANES, LANES)] = (own[g] + recv[g]) * scale

        for _, _, message in messages:
            message.wait_send()

        @pl.when(is_streamer)
        def _():
            for j in range(len(messages)):
                finish(j)
            raw.wait_send()

        @pl.when(is_helper)
        def _():
            raw.wait_recv()
            raw_acc = None
            for r in range(0, streamed, SUBLANES):
                raw_acc = merge(raw_acc, raw_buf[pl.ds(r, SUBLANES), :],
                                m - streamed + r)
            raw_row = to_row(raw_acc)
            for j in range(len(messages) - 1):
                finish(j)
            is_raw = (lax.broadcasted_iota(jnp.int32, (1, LANES), 1)
                      >= LANES - streamed)
            last_message.wait_recv()
            theirs = jnp.where(is_raw, raw_row, recv[groups - 1])
            out_ref[:, pl.ds((groups - 1) * LANES, LANES)] = (
                own[groups - 1] + theirs) * scale

    out = pl.pallas_call(
        body,
        out_shape=jax.ShapeDtypeStruct((1, m), jnp.float32),
        in_specs=[pl.BlockSpec(memory_space=pltpu.HBM)],
        out_specs=pl.BlockSpec(memory_space=pltpu.VMEM),
        scratch_shapes=[
            pltpu.VMEM((m, n), jnp.float32),
            pltpu.VMEM((streamed, n), jnp.float32),
            pltpu.VMEM((groups, 1, LANES), jnp.float32),
            pltpu.VMEM((groups, 1, LANES), jnp.float32),
            pltpu.SemaphoreType.DMA((len(CHUNKS),)),
            pltpu.SemaphoreType.DMA((len(MESSAGES),)),
            pltpu.SemaphoreType.DMA((len(MESSAGES),)),
            pltpu.SemaphoreType.DMA,
            pltpu.SemaphoreType.DMA,
        ],
        compiler_params=pltpu.CompilerParams(
            collective_id=0,
            disable_bounds_checks=True,
            disable_semaphore_checks=True,
        ),
    )(x)
    return out.reshape(m, 1)
```

```python
import jax
import jax.numpy as jnp
from jax import lax
from jax.experimental import pallas as pl
from jax.experimental.pallas import tpu as pltpu

LANES = 128
SUBLANES = 8
Y_SIZE = 2

HEAD_CHUNKS = (256, 384, 128, 72, 56)
EARLY_ROWS = 40
TAIL_ROWS = 48
STREAMED_ROWS = 40

HEAD, EARLY, TAIL, LAST, RAW = range(5)


def pallas_dist_mean_ax1_xy_m1024_n512_kernel(x: jax.Array):
    m, n = x.shape
    groups = m // LANES
    last = groups - 1
    assert n == 4 * LANES and sum(HEAD_CHUNKS) == last * LANES
    assert EARLY_ROWS + TAIL_ROWS + STREAMED_ROWS == LANES
    assert TAIL_ROWS % (2 * SUBLANES) == 0
    scale = 1.0 / (Y_SIZE * n)
    chunks = HEAD_CHUNKS + (EARLY_ROWS, TAIL_ROWS, STREAMED_ROWS)

    def body(x_hbm, out_ref, x_buf, raw_buf, sums_out, sums_in, tail_out,
             tail_in, load_sems, send_sems, recv_sems):
        loads = []
        row0 = 0
        for i, rows in enumerate(chunks):
            load = pltpu.make_async_copy(
                x_hbm.at[pl.ds(row0, rows)], x_buf.at[pl.ds(row0, rows)],
                load_sems.at[i])
            load.start(priority=int(i >= len(HEAD_CHUNKS)))
            loads.append(load)
            row0 += rows
        early_load, tail_load, streamed_load = loads[len(HEAD_CHUNKS):]

        my_y = lax.axis_index("y")
        peer = (lax.axis_index("x"), 1 - my_y)
        is_streamer = my_y == 1
        is_helper = my_y == 0
        barrier = pltpu.get_barrier_semaphore()
        pl.semaphore_signal(barrier, 1, device_id=peer,
                            device_id_type=pl.DeviceIdType.MESH)

        def to_peer(src, dst, which):
            return pltpu.make_async_remote_copy(
                src, dst, send_sems.at[which], recv_sems.at[which],
                device_id=peer, device_id_type=pl.DeviceIdType.MESH)

        head = to_peer(sums_out.at[pl.ds(0, last)], sums_in.at[pl.ds(0, last)], HEAD)
        early = to_peer(sums_out.at[last], sums_in.at[last], EARLY)
        tail = to_peer(tail_out, tail_in, TAIL)
        whole_last = to_peer(sums_out.at[groups], sums_in.at[groups], LAST)
        raw = to_peer(x_hbm.at[pl.ds(m - STREAMED_ROWS, STREAMED_ROWS)], raw_buf, RAW)

        @pl.when(is_streamer)
        def _():
            pl.semaphore_wait(barrier, 1)
            raw.start()

        lane = lax.broadcasted_iota(jnp.int32, (SUBLANES, LANES), 1)
        lane_block = lane >> 3
        lane_in_block = lane & 7

        def row_sums(block):
            folded = ((block[:, 0 * LANES:1 * LANES] + block[:, 1 * LANES:2 * LANES])
                      + (block[:, 2 * LANES:3 * LANES] + block[:, 3 * LANES:4 * LANES]))
            return jnp.broadcast_to(
                jnp.sum(folded, axis=1, keepdims=True), folded.shape)

        def merge(acc, sums, k):
            return sums if acc is None else jnp.where(lane_block == k, sums, acc)

        def to_row(acc):
            return jnp.take_along_axis(
                acc, lane_in_block, axis=0, mode="promise_in_bounds")[0:1]

        def merge_rows(acc, ref, ref_row0, rows, first_block):
            for k in range(rows // SUBLANES):
                block = ref[pl.ds(ref_row0 + k * SUBLANES, SUBLANES), :]
                acc = merge(acc, row_sums(block), first_block + k)
            return acc

        own = []
        acc = None
        row0 = 0
        for load, rows in zip(loads, HEAD_CHUNKS):
            load.wait()
            for r in range(row0, row0 + rows, SUBLANES):
                acc = merge_rows(acc, x_buf, r, SUBLANES, r % LANES // SUBLANES)
                if (r + SUBLANES) % LANES == 0:
                    own.append(to_row(acc))
                    sums_out[r // LANES] = own[-1]
                    acc = None
            row0 += rows

        @pl.when(is_helper)
        def _():
            pl.semaphore_wait(barrier, 1)

        head.start()

        early_load.wait()
        acc = merge_rows(None, x_buf, row0, EARLY_ROWS, 0)
        sums_out[last] = to_row(acc)
        early.start()
        row0 += EARLY_ROWS

        tail_load.wait()
        tail_sums = [
            row_sums(x_buf[pl.ds(r, 2 * SUBLANES), :])
            for r in range(row0, row0 + TAIL_ROWS, 2 * SUBLANES)]
        words = None
        for k, sums in enumerate(tail_sums):
            words = merge(
                words, pltpu.bitcast(sums.astype(jnp.bfloat16), jnp.int32), k)
        tail_out[...] = to_row(words)
        tail.start()
        for k, sums in enumerate(tail_sums):
            block = EARLY_ROWS // SUBLANES + 2 * k
            acc = merge(acc, sums[:SUBLANES], block)
            acc = merge(acc, sums[SUBLANES:], block + 1)
        row0 += TAIL_ROWS

        streamed_load.wait()
        first_streamed = LANES - STREAMED_ROWS
        acc = merge_rows(acc, x_buf, row0, STREAMED_ROWS, first_streamed // SUBLANES)
        own_last = to_row(acc)

        @pl.when(is_helper)
        def _():
            sums_out[groups] = own_last
            whole_last.start()

        def finish_head():
            head.wait_recv()
            for g in range(last):
                out_ref[:, pl.ds(g * LANES, LANES)] = (own[g] + sums_in[g]) * scale

        head.wait_send()
        early.wait_send()
        tail.wait_send()

        @pl.when(is_streamer)
        def _():
            finish_head()
            early.wait_recv()
            tail.wait_recv()
            raw.wait_send()
            whole_last.wait_recv()
            out_ref[:, pl.ds(last * LANES, LANES)] = (own_last + sums_in[groups]) * scale

        @pl.when(is_helper)
        def _():
            whole_last.wait_send()
            raw.wait_recv()
            streamed = to_row(merge_rows(
                None, raw_buf, 0, STREAMED_ROWS, first_streamed // SUBLANES))
            finish_head()
            row = lax.broadcasted_iota(jnp.int32, (1, LANES), 1)
            early.wait_recv()
            known = own_last + jnp.where(
                row >= first_streamed, streamed,
                jnp.where(row < EARLY_ROWS, sums_in[last], 0.0))
            tail_row = row - EARLY_ROWS
            word_index = tail_row >> 1
            shift = (1 - (tail_row & 1)) << 4
            word = jnp.zeros((1, LANES), jnp.int32)
            tail.wait_recv()
            for j in range(TAIL_ROWS // 2):
                word = jnp.where(word_index == j, tail_in[0, j], word)
            tail_sum = pltpu.bitcast((word << shift) & jnp.int32(-65536), jnp.float32)
            out_ref[:, pl.ds(last * LANES, LANES)] = (known + tail_sum) * scale

    out = pl.pallas_call(
        body,
        out_shape=jax.ShapeDtypeStruct((1, m), jnp.float32),
        in_specs=[pl.BlockSpec(memory_space=pltpu.HBM)],
        out_specs=pl.BlockSpec(memory_space=pltpu.VMEM),
        scratch_shapes=[
            pltpu.VMEM((m, n), jnp.float32),
            pltpu.VMEM((STREAMED_ROWS, n), jnp.float32),
            pltpu.VMEM((groups + 1, 1, LANES), jnp.float32),
            pltpu.VMEM((groups + 1, 1, LANES), jnp.float32),
            pltpu.VMEM((1, LANES), jnp.int32),
            pltpu.SMEM((1, LANES), jnp.int32),
            pltpu.SemaphoreType.DMA((len(chunks),)),
            pltpu.SemaphoreType.DMA((5,)),
            pltpu.SemaphoreType.DMA((5,)),
        ],
        compiler_params=pltpu.CompilerParams(
            collective_id=0,
            disable_bounds_checks=True,
            disable_semaphore_checks=True,
        ),
    )(x)
    return out.reshape(m, 1)
```

```python
import jax
import jax.numpy as jnp
from jax import lax
from jax.experimental import pallas as pl
from jax.experimental.pallas import tpu as pltpu

LANES = 128
SUBLANES = 8
Y_SIZE = 2

HEAD_CHUNKS = (256, 384, 128, 72, 56)
EARLY_ROWS = 40
TAIL_CHUNKS = (32, 16)
STREAMED_ROWS = 40
TAIL_ROWS = sum(TAIL_CHUNKS)

HEAD, EARLY, TAIL, LAST, RAW = range(5)


def pallas_dist_mean_ax1_xy_m1024_n512_kernel(x: jax.Array):
    m, n = x.shape
    groups = m // LANES
    last = groups - 1
    assert n == 4 * LANES and sum(HEAD_CHUNKS) == last * LANES
    assert EARLY_ROWS + TAIL_ROWS + STREAMED_ROWS == LANES
    assert all(rows % (2 * SUBLANES) == 0 for rows in TAIL_CHUNKS)
    scale = 1.0 / (Y_SIZE * n)
    chunks = HEAD_CHUNKS + (EARLY_ROWS,) + TAIL_CHUNKS + (STREAMED_ROWS,)

    def body(x_hbm, out_ref, x_buf, raw_buf, sums_out, sums_in, tail_out,
             tail_in, load_sems, send_sems, recv_sems):
        loads = []
        row0 = 0
        for i, rows in enumerate(chunks):
            load = pltpu.make_async_copy(
                x_hbm.at[pl.ds(row0, rows)], x_buf.at[pl.ds(row0, rows)],
                load_sems.at[i])
            load.start(priority=min(i, 1))
            loads.append(load)
            row0 += rows
        early_load, *tail_loads, streamed_load = loads[len(HEAD_CHUNKS):]

        my_y = lax.axis_index("y")
        peer = (lax.axis_index("x"), 1 - my_y)
        is_streamer = my_y == 1
        is_helper = my_y == 0
        barrier = pltpu.get_barrier_semaphore()
        pl.semaphore_signal(barrier, 1, device_id=peer,
                            device_id_type=pl.DeviceIdType.MESH)

        def to_peer(src, dst, which):
            return pltpu.make_async_remote_copy(
                src, dst, send_sems.at[which], recv_sems.at[which],
                device_id=peer, device_id_type=pl.DeviceIdType.MESH)

        head = to_peer(sums_out.at[pl.ds(0, last)], sums_in.at[pl.ds(0, last)], HEAD)
        early = to_peer(sums_out.at[last], sums_in.at[last], EARLY)
        tail = to_peer(tail_out, tail_in, TAIL)
        whole_last = to_peer(sums_out.at[groups], sums_in.at[groups], LAST)
        raw = to_peer(x_hbm.at[pl.ds(m - STREAMED_ROWS, STREAMED_ROWS)], raw_buf, RAW)

        @pl.when(is_streamer)
        def _():
            pl.semaphore_wait(barrier, 1)
            raw.start()

        lane = lax.broadcasted_iota(jnp.int32, (SUBLANES, LANES), 1)
        lane_block = lane >> 3
        lane_in_block = lane & 7

        def fold(block):
            return ((block[:, 0 * LANES:1 * LANES] + block[:, 1 * LANES:2 * LANES])
                    + (block[:, 2 * LANES:3 * LANES] + block[:, 3 * LANES:4 * LANES]))

        def lane_sum(folded):
            return jnp.broadcast_to(
                jnp.sum(folded, axis=1, keepdims=True), folded.shape)

        def merge(acc, sums, k):
            return sums if acc is None else jnp.where(lane_block == k, sums, acc)

        def to_row(acc):
            return jnp.take_along_axis(
                acc, lane_in_block, axis=0, mode="promise_in_bounds")[0:1]

        def merge_rows(acc, ref, ref_row0, rows, first_block):
            for k in range(rows // SUBLANES):
                block = ref[pl.ds(ref_row0 + k * SUBLANES, SUBLANES), :]
                acc = merge(acc, lane_sum(fold(block)), first_block + k)
            return acc

        own = []
        acc = None
        row0 = 0
        for load, rows in zip(loads, HEAD_CHUNKS):
            load.wait()
            for r in range(row0, row0 + rows, SUBLANES):
                acc = merge_rows(acc, x_buf, r, SUBLANES, r % LANES // SUBLANES)
                if (r + SUBLANES) % LANES == 0:
                    own.append(to_row(acc))
                    sums_out[r // LANES] = own[-1]
                    acc = None
            row0 += rows

        @pl.when(is_helper)
        def _():
            pl.semaphore_wait(barrier, 1)

        head.start()

        early_load.wait()
        acc = merge_rows(None, x_buf, row0, EARLY_ROWS, 0)
        sums_out[last] = to_row(acc)
        early.start()
        row0 += EARLY_ROWS

        folded = []
        for load, rows in zip(tail_loads, TAIL_CHUNKS):
            load.wait()
            folded += [fold(x_buf[pl.ds(r, 2 * SUBLANES), :])
                       for r in range(row0, row0 + rows, 2 * SUBLANES)]
            row0 += rows
        tail_sums = [lane_sum(f) for f in folded]
        words = None
        for k, sums in enumerate(tail_sums):
            words = merge(
                words, pltpu.bitcast(sums.astype(jnp.bfloat16), jnp.int32), k)
        tail_out[...] = to_row(words)
        tail.start()
        for k, sums in enumerate(tail_sums):
            block = EARLY_ROWS // SUBLANES + 2 * k
            acc = merge(acc, sums[:SUBLANES], block)
            acc = merge(acc, sums[SUBLANES:], block + 1)

        streamed_load.wait()
        first_streamed = LANES - STREAMED_ROWS
        acc = merge_rows(acc, x_buf, row0, STREAMED_ROWS, first_streamed // SUBLANES)
        own_last = to_row(acc)

        @pl.when(is_helper)
        def _():
            sums_out[groups] = own_last
            whole_last.start()

        def finish_head():
            head.wait_recv()
            for g in range(last):
                out_ref[:, pl.ds(g * LANES, LANES)] = (own[g] + sums_in[g]) * scale

        head.wait_send()
        early.wait_send()
        tail.wait_send()

        @pl.when(is_streamer)
        def _():
            finish_head()
            early.wait_recv()
            tail.wait_recv()
            raw.wait_send()
            whole_last.wait_recv()
            out_ref[:, pl.ds(last * LANES, LANES)] = (own_last + sums_in[groups]) * scale

        @pl.when(is_helper)
        def _():
            whole_last.wait_send()
            raw.wait_recv()
            streamed = to_row(merge_rows(
                None, raw_buf, 0, STREAMED_ROWS, first_streamed // SUBLANES))
            finish_head()
            row = lax.broadcasted_iota(jnp.int32, (1, LANES), 1)
            early.wait_recv()
            known = own_last + jnp.where(
                row >= first_streamed, streamed,
                jnp.where(row < EARLY_ROWS, sums_in[last], 0.0))
            tail_row = row - EARLY_ROWS
            word_index = tail_row >> 1
            shift = (1 - (tail_row & 1)) << 4
            word = jnp.zeros((1, LANES), jnp.int32)
            tail.wait_recv()
            for j in range(TAIL_ROWS // 2):
                word = jnp.where(word_index == j, tail_in[0, j], word)
            tail_sum = pltpu.bitcast((word << shift) & jnp.int32(-65536), jnp.float32)
            out_ref[:, pl.ds(last * LANES, LANES)] = (known + tail_sum) * scale

    out = pl.pallas_call(
        body,
        out_shape=jax.ShapeDtypeStruct((1, m), jnp.float32),
        in_specs=[pl.BlockSpec(memory_space=pltpu.HBM)],
        out_specs=pl.BlockSpec(memory_space=pltpu.VMEM),
        scratch_shapes=[
            pltpu.VMEM((m, n), jnp.float32),
            pltpu.VMEM((STREAMED_ROWS, n), jnp.float32),
            pltpu.VMEM((groups + 1, 1, LANES), jnp.float32),
            pltpu.VMEM((groups + 1, 1, LANES), jnp.float32),
            pltpu.VMEM((1, LANES), jnp.int32),
            pltpu.SMEM((1, LANES), jnp.int32),
            pltpu.SemaphoreType.DMA((len(chunks),)),
            pltpu.SemaphoreType.DMA((5,)),
            pltpu.SemaphoreType.DMA((5,)),
        ],
        compiler_params=pltpu.CompilerParams(
            collective_id=0, disable_semaphore_checks=True),
    )(x)
    return out.reshape(m, 1)
```

```python
import jax
import jax.numpy as jnp
from jax import lax
from jax.experimental import pallas as pl
from jax.experimental.pallas import tpu as pltpu

LANES = 128
SUBLANES = 8
Y_SIZE = 2

HEAD_CHUNKS = (16, 240, 384, 128, 72, 56)
EARLY_ROWS = 40
TAIL_CHUNKS = (32, 16)
STREAMED_ROWS = 40
TAIL_ROWS = sum(TAIL_CHUNKS)

HEAD, EARLY, TAIL, LAST, RAW = range(5)


def pallas_dist_mean_ax1_xy_m1024_n512_kernel(x: jax.Array):
    m, n = x.shape
    groups = m // LANES
    last = groups - 1
    assert n == 4 * LANES and sum(HEAD_CHUNKS) == last * LANES
    assert EARLY_ROWS + TAIL_ROWS + STREAMED_ROWS == LANES
    assert all(rows % (2 * SUBLANES) == 0 for rows in TAIL_CHUNKS)
    scale = 1.0 / (Y_SIZE * n)
    chunks = HEAD_CHUNKS + (EARLY_ROWS,) + TAIL_CHUNKS + (STREAMED_ROWS,)

    def body(x_hbm, out_ref, x_buf, raw_buf, sums_out, sums_in, tail_out,
             tail_in, load_sems, send_sems, recv_sems):
        loads = []
        row0 = 0
        for i, rows in enumerate(chunks):
            load = pltpu.make_async_copy(
                x_hbm.at[pl.ds(row0, rows)], x_buf.at[pl.ds(row0, rows)],
                load_sems.at[i])
            load.start(priority=min(i, 1))
            loads.append(load)
            row0 += rows
        early_load, *tail_loads, streamed_load = loads[len(HEAD_CHUNKS):]

        my_y = lax.axis_index("y")
        peer = (lax.axis_index("x"), 1 - my_y)
        is_streamer = my_y == 1
        is_helper = my_y == 0
        barrier = pltpu.get_barrier_semaphore()
        pl.semaphore_signal(barrier, 1, device_id=peer,
                            device_id_type=pl.DeviceIdType.MESH)

        def to_peer(src, dst, which):
            return pltpu.make_async_remote_copy(
                src, dst, send_sems.at[which], recv_sems.at[which],
                device_id=peer, device_id_type=pl.DeviceIdType.MESH)

        head = to_peer(sums_out.at[pl.ds(0, last)], sums_in.at[pl.ds(0, last)], HEAD)
        early = to_peer(sums_out.at[last], sums_in.at[last], EARLY)
        tail = to_peer(tail_out, tail_in, TAIL)
        whole_last = to_peer(sums_out.at[groups], sums_in.at[groups], LAST)
        raw = to_peer(x_hbm.at[pl.ds(m - STREAMED_ROWS, STREAMED_ROWS)], raw_buf, RAW)

        pl.semaphore_wait(barrier, 1)

        @pl.when(is_streamer)
        def _():
            raw.start()

        lane = lax.broadcasted_iota(jnp.int32, (SUBLANES, LANES), 1)
        lane_block = lane >> 3
        lane_in_block = lane & 7

        def fold(block):
            return ((block[:, 0 * LANES:1 * LANES] + block[:, 1 * LANES:2 * LANES])
                    + (block[:, 2 * LANES:3 * LANES] + block[:, 3 * LANES:4 * LANES]))

        def lane_sum(folded):
            return jnp.broadcast_to(
                jnp.sum(folded, axis=1, keepdims=True), folded.shape)

        def merge(acc, sums, k):
            return sums if acc is None else jnp.where(lane_block == k, sums, acc)

        def to_row(acc):
            return jnp.take_along_axis(
                acc, lane_in_block, axis=0, mode="promise_in_bounds")[0:1]

        def merge_rows(acc, ref, ref_row0, rows, first_block):
            for k in range(rows // SUBLANES):
                block = ref[pl.ds(ref_row0 + k * SUBLANES, SUBLANES), :]
                acc = merge(acc, lane_sum(fold(block)), first_block + k)
            return acc

        own = []
        acc = None
        row0 = 0
        for load, rows in zip(loads, HEAD_CHUNKS):
            load.wait()
            for r in range(row0, row0 + rows, SUBLANES):
                acc = merge_rows(acc, x_buf, r, SUBLANES, r % LANES // SUBLANES)
                if (r + SUBLANES) % LANES == 0:
                    own.append(to_row(acc))
                    sums_out[r // LANES] = own[-1]
                    acc = None
            row0 += rows

        head.start()

        early_load.wait()
        acc = merge_rows(None, x_buf, row0, EARLY_ROWS, 0)
        sums_out[last] = to_row(acc)
        early.start()
        row0 += EARLY_ROWS

        folded = []
        for load, rows in zip(tail_loads, TAIL_CHUNKS):
            load.wait()
            folded += [fold(x_buf[pl.ds(r, 2 * SUBLANES), :])
                       for r in range(row0, row0 + rows, 2 * SUBLANES)]
            row0 += rows
        words = None
        for k, block in enumerate(folded):
            pairs = lane_sum(block).astype(jnp.bfloat16)
            words = merge(words, pltpu.bitcast(pairs, jnp.int32), k)
        tail_out[...] = to_row(words)
        tail.start()

        streamed_load.wait()
        own_last = to_row(merge_rows(
            acc, x_buf, last * LANES + EARLY_ROWS, LANES - EARLY_ROWS,
            EARLY_ROWS // SUBLANES))

        @pl.when(is_helper)
        def _():
            sums_out[groups] = own_last
            whole_last.start()

        def finish_head():
            head.wait_recv()
            for g in range(last):
                out_ref[:, pl.ds(g * LANES, LANES)] = (own[g] + sums_in[g]) * scale

        head.wait_send()
        early.wait_send()
        tail.wait_send()

        @pl.when(is_streamer)
        def _():
            finish_head()
            early.wait_recv()
            tail.wait_recv()
            raw.wait_send()
            whole_last.wait_recv()
            out_ref[:, pl.ds(last * LANES, LANES)] = (own_last + sums_in[groups]) * scale

        @pl.when(is_helper)
        def _():
            whole_last.wait_send()
            raw.wait_recv()
            first_streamed = LANES - STREAMED_ROWS
            streamed = to_row(merge_rows(
                None, raw_buf, 0, STREAMED_ROWS, first_streamed // SUBLANES))
            finish_head()
            row = lax.broadcasted_iota(jnp.int32, (1, LANES), 1)
            early.wait_recv()
            known = own_last + jnp.where(
                row >= first_streamed, streamed,
                jnp.where(row < EARLY_ROWS, sums_in[last], 0.0))
            tail_row = row - EARLY_ROWS
            word_index = tail_row >> 1
            shift = (1 - (tail_row & 1)) << 4
            word = jnp.zeros((1, LANES), jnp.int32)
            tail.wait_recv()
            for j in range(TAIL_ROWS // 2):
                word = jnp.where(word_index == j, tail_in[0, j], word)
            tail_sum = pltpu.bitcast((word << shift) & jnp.int32(-65536), jnp.float32)
            out_ref[:, pl.ds(last * LANES, LANES)] = (known + tail_sum) * scale

    out = pl.pallas_call(
        body,
        out_shape=jax.ShapeDtypeStruct((1, m), jnp.float32),
        in_specs=[pl.BlockSpec(memory_space=pltpu.HBM)],
        out_specs=pl.BlockSpec(memory_space=pltpu.VMEM),
        scratch_shapes=[
            pltpu.VMEM((m, n), jnp.float32),
            pltpu.VMEM((STREAMED_ROWS, n), jnp.float32),
            pltpu.VMEM((groups + 1, 1, LANES), jnp.float32),
            pltpu.VMEM((groups + 1, 1, LANES), jnp.float32),
            pltpu.VMEM((1, LANES), jnp.int32),
            pltpu.SMEM((1, LANES), jnp.int32),
            pltpu.SemaphoreType.DMA((len(chunks),)),
            pltpu.SemaphoreType.DMA((5,)),
            pltpu.SemaphoreType.DMA((5,)),
        ],
        compiler_params=pltpu.CompilerParams(
            collective_id=0, disable_semaphore_checks=True),
    )(x)
    return out.reshape(m, 1)
```

```python
import jax
import jax.numpy as jnp
from jax import lax
from jax.experimental import pallas as pl
from jax.experimental.pallas import tpu as pltpu

LANES = 128
SUBLANES = 8
Y_SIZE = 2

HEAD_CHUNKS = (16, 240, 384, 128, 72, 56)
EARLY_ROWS = 48
TAIL_CHUNKS = (32, 8)
STREAMED_ROWS = 40
TAIL_ROWS = sum(TAIL_CHUNKS)

HEAD, EARLY, TAIL, LAST, RAW = range(5)


def pallas_dist_mean_ax1_xy_m1024_n512_kernel(x: jax.Array):
    m, n = x.shape
    groups = m // LANES
    last = groups - 1
    assert n == 4 * LANES and sum(HEAD_CHUNKS) == last * LANES
    assert EARLY_ROWS + TAIL_ROWS + STREAMED_ROWS == LANES
    scale = 1.0 / (Y_SIZE * n)
    chunks = HEAD_CHUNKS + (EARLY_ROWS,) + TAIL_CHUNKS + (STREAMED_ROWS,)

    def body(x_hbm, out_ref, x_buf, raw_buf, sums_out, sums_in, tail_out,
             tail_in, load_sems, send_sems, recv_sems):
        loads = []
        row0 = 0
        for i, rows in enumerate(chunks):
            load = pltpu.make_async_copy(
                x_hbm.at[pl.ds(row0, rows)], x_buf.at[pl.ds(row0, rows)],
                load_sems.at[i])
            load.start(priority=min(i, 1))
            loads.append(load)
            row0 += rows
        early_load, *tail_loads, streamed_load = loads[len(HEAD_CHUNKS):]

        my_y = lax.axis_index("y")
        peer = (lax.axis_index("x"), 1 - my_y)
        is_streamer = my_y == 1
        is_helper = my_y == 0
        barrier = pltpu.get_barrier_semaphore()
        pl.semaphore_signal(barrier, 1, device_id=peer,
                            device_id_type=pl.DeviceIdType.MESH)

        def to_peer(src, dst, which):
            return pltpu.make_async_remote_copy(
                src, dst, send_sems.at[which], recv_sems.at[which],
                device_id=peer, device_id_type=pl.DeviceIdType.MESH)

        head = to_peer(sums_out.at[pl.ds(0, last)], sums_in.at[pl.ds(0, last)], HEAD)
        early = to_peer(sums_out.at[last], sums_in.at[last], EARLY)
        tail = to_peer(tail_out, tail_in, TAIL)
        whole_last = to_peer(sums_out.at[groups], sums_in.at[groups], LAST)
        raw = to_peer(x_hbm.at[pl.ds(m - STREAMED_ROWS, STREAMED_ROWS)], raw_buf, RAW)

        pl.semaphore_wait(barrier, 1)

        @pl.when(is_streamer)
        def _():
            raw.start()

        lane = lax.broadcasted_iota(jnp.int32, (SUBLANES, LANES), 1)
        lane_block = lane >> 3
        lane_in_block = lane & 7

        def fold(block):
            return ((block[:, 0 * LANES:1 * LANES] + block[:, 1 * LANES:2 * LANES])
                    + (block[:, 2 * LANES:3 * LANES] + block[:, 3 * LANES:4 * LANES]))

        def lane_sum(folded):
            return jnp.broadcast_to(
                jnp.sum(folded, axis=1, keepdims=True), folded.shape)

        def merge(acc, sums, k):
            return sums if acc is None else jnp.where(lane_block == k, sums, acc)

        def to_row(acc):
            return jnp.take_along_axis(
                acc, lane_in_block, axis=0, mode="promise_in_bounds")[0:1]

        def merge_rows(acc, ref, ref_row0, rows, first_block):
            for k in range(rows // SUBLANES):
                block = ref[pl.ds(ref_row0 + k * SUBLANES, SUBLANES), :]
                acc = merge(acc, lane_sum(fold(block)), first_block + k)
            return acc

        own = []
        acc = None
        row0 = 0
        for load, rows in zip(loads, HEAD_CHUNKS):
            load.wait()
            for r in range(row0, row0 + rows, SUBLANES):
                acc = merge_rows(acc, x_buf, r, SUBLANES, r % LANES // SUBLANES)
                if (r + SUBLANES) % LANES == 0:
                    own.append(to_row(acc))
                    sums_out[r // LANES] = own[-1]
                    acc = None
            row0 += rows

        head.start()

        early_load.wait()
        acc = merge_rows(None, x_buf, row0, EARLY_ROWS, 0)
        sums_out[last] = to_row(acc)
        early.start()
        row0 += EARLY_ROWS

        folded = []
        for load, rows in zip(tail_loads, TAIL_CHUNKS):
            load.wait()
            folded += [fold(x_buf[pl.ds(r, SUBLANES), :])
                       for r in range(row0, row0 + rows, SUBLANES)]
            row0 += rows
        halves = [None, None]
        for k, block in enumerate(folded):
            halves[k % 2] = merge(halves[k % 2], lane_sum(block), k // 2)
        words = pltpu.bitcast(
            jnp.concatenate(halves, axis=0).astype(jnp.bfloat16), jnp.int32)
        tail_out[...] = to_row(words)
        tail.start()

        streamed_load.wait()
        own_last = to_row(merge_rows(
            acc, x_buf, last * LANES + EARLY_ROWS, LANES - EARLY_ROWS,
            EARLY_ROWS // SUBLANES))

        @pl.when(is_helper)
        def _():
            sums_out[groups] = own_last
            whole_last.start()

        def finish_head():
            head.wait_recv()
            for g in range(last):
                out_ref[:, pl.ds(g * LANES, LANES)] = (own[g] + sums_in[g]) * scale

        head.wait_send()
        early.wait_send()
        tail.wait_send()

        @pl.when(is_streamer)
        def _():
            finish_head()
            early.wait_recv()
            tail.wait_recv()
            raw.wait_send()
            whole_last.wait_recv()
            out_ref[:, pl.ds(last * LANES, LANES)] = (own_last + sums_in[groups]) * scale

        @pl.when(is_helper)
        def _():
            whole_last.wait_send()
            raw.wait_recv()
            first_streamed = LANES - STREAMED_ROWS
            streamed = to_row(merge_rows(
                None, raw_buf, 0, STREAMED_ROWS, first_streamed // SUBLANES))
            finish_head()
            row = lax.broadcasted_iota(jnp.int32, (1, LANES), 1)
            early.wait_recv()
            known = own_last + jnp.where(
                row >= first_streamed, streamed,
                jnp.where(row < EARLY_ROWS, sums_in[last], 0.0))
            tail_row = row - EARLY_ROWS
            word_index = tail_row >> 1
            shift = (1 - (tail_row & 1)) << 4
            word = jnp.zeros((1, LANES), jnp.int32)
            tail.wait_recv()
            for j in range(TAIL_ROWS // 2):
                word = jnp.where(word_index == j, tail_in[0, j], word)
            tail_sum = pltpu.bitcast((word << shift) & jnp.int32(-65536), jnp.float32)
            out_ref[:, pl.ds(last * LANES, LANES)] = (known + tail_sum) * scale

    out = pl.pallas_call(
        body,
        out_shape=jax.ShapeDtypeStruct((1, m), jnp.float32),
        in_specs=[pl.BlockSpec(memory_space=pltpu.HBM)],
        out_specs=pl.BlockSpec(memory_space=pltpu.VMEM),
        scratch_shapes=[
            pltpu.VMEM((m, n), jnp.float32),
            pltpu.VMEM((STREAMED_ROWS, n), jnp.float32),
            pltpu.VMEM((groups + 1, 1, LANES), jnp.float32),
            pltpu.VMEM((groups + 1, 1, LANES), jnp.float32),
            pltpu.VMEM((1, LANES), jnp.int32),
            pltpu.SMEM((1, LANES), jnp.int32),
            pltpu.SemaphoreType.DMA((len(chunks),)),
            pltpu.SemaphoreType.DMA((5,)),
            pltpu.SemaphoreType.DMA((5,)),
        ],
        compiler_params=pltpu.CompilerParams(
            collective_id=0, disable_semaphore_checks=True),
    )(x)
    return out.reshape(m, 1)
```
